```python
import numpy as np

kernel_name = "dist_rsx_agy_m2048_n1024"

def setup_inputs():
    return {"x": np.random.randn(2, 2048, 2048).astype(np.float32)}

def reference(x: np.ndarray) -> np.ndarray:
    return x.sum(axis=0)
```

```python
import jax
import jax.numpy as jnp
from jax import lax
from jax.experimental import pallas as pl
from jax.experimental.pallas import tpu as pltpu

_MESH = pl.DeviceIdType.MESH
_ROWS = 16
_AHEAD = 6
_TAIL = 1
_LOAD_EDGES = (0, 16, 64, 256, 1024)


def pallas_dist_rsx_agy_m2048_n1024_kernel(x: jax.Array):
    _, m, cols = x.shape
    half = m // 2
    n = half // _ROWS
    blocks = list(zip(_LOAD_EDGES[:-1], _LOAD_EDGES[1:]))

    def body(x_hbm, out, xs, xo, sx, rx, ld_sem, raw_sem, sum_sem, misc_sem):
        mx = lax.axis_index("x")
        my = lax.axis_index("y")
        xn = (1 - mx, my)
        yn = (mx, 1 - my)
        bar = pltpu.get_barrier_semaphore()
        pl.semaphore_signal(bar, 1, device_id=xn, device_id_type=_MESH)
        pl.semaphore_signal(bar, 1, device_id=yn, device_id_type=_MESH)

        own0 = pl.multiple_of(mx * half, half)
        oth0 = pl.multiple_of((1 - mx) * half, half)
        myc = pl.ds(pl.multiple_of(my * cols, cols), cols)
        otc = pl.ds(pl.multiple_of((1 - my) * cols, cols), cols)
        send_x, send_y, fin, yfw = (misc_sem.at[i] for i in range(4))

        ld_s = [pltpu.make_async_copy(x_hbm.at[0, pl.ds(oth0 + a, b - a), :], xs.at[pl.ds(a, b - a), :],
                                      ld_sem.at[0, i]) for i, (a, b) in enumerate(blocks)]
        ld_o = [pltpu.make_async_copy(x_hbm.at[0, pl.ds(own0 + a, b - a), :], xo.at[pl.ds(a, b - a), :],
                                      ld_sem.at[1, i]) for i, (a, b) in enumerate(blocks)]
        for i in range(len(blocks)):
            ld_s[i].start()
            ld_o[i].start()

        def rdma(src, dst, ssem, rsem, dev):
            return pltpu.make_async_remote_copy(src, dst, ssem, rsem, device_id=dev, device_id_type=_MESH)

        def raw(k):
            r = pl.ds(k * _ROWS, _ROWS)
            return rdma(sx.at[r, :], rx.at[r, :], send_x, raw_sem.at[k], xn)

        def own_blk(k):
            return out.at[pl.ds(own0 + k * _ROWS, _ROWS), myc]

        def oth_blk(k):
            return out.at[pl.ds(oth0 + k * _ROWS, _ROWS), myc]

        waited_s, waited_o = set(), set()

        def need(waited, lds, k):
            for i, (a, b) in enumerate(blocks):
                if a < (k + 1) * _ROWS and b > k * _ROWS and i not in waited:
                    lds[i].wait()
                    waited.add(i)

        def x_send(j):
            if j < n:
                need(waited_s, ld_s, j)
                r = pl.ds(j * _ROWS, _ROWS)
                sx[r, :] = xs[r, :].astype(jnp.bfloat16)
                if j == 0:
                    pl.semaphore_wait(bar, 2)
                raw(j).start()
            elif j < 2 * n - _TAIL:
                k = j - n
                rdma(own_blk(k), own_blk(k), send_x, sum_sem.at[k], xn).start()
            elif j == 2 * n - _TAIL:
                t = out.at[pl.ds(own0 + (n - _TAIL) * _ROWS, _TAIL * _ROWS), myc]
                rdma(t, t, send_x, fin, xn).start()
                t = out.at[pl.ds(own0 + (n - _TAIL) * _ROWS, _TAIL * _ROWS), otc]
                rdma(t, t, send_x, yfw, yn).wait_recv()
                rdma(t, t, send_x, fin, xn).start()

        for j in range(_AHEAD):
            x_send(j)
        for k in range(n):
            need(waited_o, ld_o, k)
            raw(k).wait_recv()
            r = pl.ds(k * _ROWS, _ROWS)
            s = xo[r, :] + rx[r, :].astype(jnp.float32)
            out[pl.ds(own0 + k * _ROWS, _ROWS), myc] = s.astype(jnp.bfloat16)
            rdma(own_blk(k), own_blk(k), send_y, fin if k < n - _TAIL else yfw, yn).start()
            x_send(k + _AHEAD)
        for k in range(n - _TAIL):
            rdma(oth_blk(k), oth_blk(k), send_x, sum_sem.at[k], xn).wait_recv()
            rdma(oth_blk(k), oth_blk(k), send_y, fin, yn).start()
            x_send(n + k + _AHEAD)

        whole = out.at[:, pl.ds(0, cols)]
        rdma(whole, whole, send_x, fin, xn).wait_recv()
        rdma(whole, whole, send_x, fin, xn).wait_send()
        t = out.at[pl.ds(0, _TAIL * _ROWS), pl.ds(0, cols)]
        rdma(t, t, send_x, fin, xn).wait_send()
        t = out.at[pl.ds(0, m - _TAIL * _ROWS), pl.ds(0, cols)]
        rdma(t, t, send_y, fin, yn).wait_send()

    return pl.pallas_call(
        body,
        out_shape=pltpu.VMEM((m, 2 * cols), jnp.bfloat16),
        in_specs=[pl.BlockSpec(memory_space=pltpu.HBM)],
        out_specs=pl.BlockSpec(memory_space=pltpu.VMEM),
        scratch_shapes=[
            pltpu.VMEM((half, cols), jnp.float32),
            pltpu.VMEM((half, cols), jnp.float32),
            pltpu.VMEM((half, cols), jnp.bfloat16),
            pltpu.VMEM((half, cols), jnp.bfloat16),
            pltpu.SemaphoreType.DMA((2, len(blocks))),
            pltpu.SemaphoreType.DMA((n,)),
            pltpu.SemaphoreType.DMA((n,)),
            pltpu.SemaphoreType.DMA((4,)),
        ],
        compiler_params=pltpu.CompilerParams(
            collective_id=0, vmem_limit_bytes=48 * 1024 * 1024, disable_semaphore_checks=True),
    )(x)
```

```python
import jax
import jax.numpy as jnp
from jax import lax
from jax.experimental import pallas as pl
from jax.experimental.pallas import tpu as pltpu

_ROWS = 8
_AHEAD = 10
_TAIL = 3
_PARTS = 4
_LOADS = (
    (False, 0, 8), (False, 8, 32), (False, 32, 96), (True, 0, 64),
    (False, 96, 256), (True, 64, 256), (False, 256, 512), (True, 256, 512),
    (False, 512, 768), (True, 512, 768), (False, 768, 1024), (True, 768, 1024),
)


def pallas_dist_rsx_agy_m2048_n1024_kernel(x: jax.Array):
    _, m, n = x.shape
    half = m // 2
    part = m // _PARTS
    share = part // 2
    chunks = half // _ROWS
    body_chunks = chunks - _TAIL

    def kernel(x_hbm, *refs):
        outs = refs[:_PARTS]
        (theirs, mine, raw_out, raw_in,
         load_sems, raw_sems, sum_sems, part_sems, sems, y_ready) = refs[_PARTS:]
        my_x, my_y = lax.axis_index("x"), lax.axis_index("y")
        x_peer, y_peer = (1 - my_x, my_y), (my_x, 1 - my_y)
        odd = my_x ^ my_y

        def signal(sem, peer):
            pl.semaphore_signal(
                sem, 1, device_id=peer, device_id_type=pl.DeviceIdType.MESH
            )

        def remote(src, dst, send_sem, recv_sem, peer):
            return pltpu.make_async_remote_copy(
                src, dst, send_sem, recv_sem, peer, pl.DeviceIdType.MESH
            )

        def wait_sent(block, sem):
            remote(block, block, sem, sem, x_peer).wait_send()

        def wait_received(block, sem):
            remote(block, block, sem, sem, x_peer).wait_recv()

        barrier = pltpu.get_barrier_semaphore()
        signal(barrier, x_peer)
        pl.when(odd == 1)(lambda: signal(barrier, y_peer))

        def first_row(owner):
            return pl.multiple_of(owner * share, share)

        def block(owner, column_half, row, rows=_ROWS):
            return outs[row // share].at[
                pl.ds(first_row(owner) + row % share, rows),
                pl.ds(pl.multiple_of(column_half * n, n), n),
            ]

        loads = []
        for i, (is_mine, lo, hi) in enumerate(_LOADS):
            row = lo // share * part + first_row(my_x if is_mine else 1 - my_x) + lo % share
            load = pltpu.make_async_copy(
                x_hbm.at[0, pl.ds(row, hi - lo), :],
                (mine if is_mine else theirs).at[pl.ds(lo, hi - lo), :],
                load_sems.at[i],
            )
            load.start()
            loads.append(load)

        def wait_loaded(is_mine, k):
            for load, (load_is_mine, lo, _) in zip(loads, _LOADS):
                if load_is_mine == is_mine and lo == k * _ROWS:
                    load.wait()

        raw_sent, tail_sent, tail_over_y, tail_own, tail_diag = (
            sems.at[i] for i in range(5)
        )
        own_x_sent, own_y_sent, diag_sent, own_received, diag_received = (
            [part_sems.at[i, p] for p in range(_PARTS)] for i in range(5)
        )
        tail_row, tail_rows = body_chunks * _ROWS, _TAIL * _ROWS

        def raw_copy(k):
            rows = pl.ds(k * _ROWS, _ROWS)
            return remote(
                raw_out.at[rows, :], raw_in.at[rows, :], raw_sent, raw_sems.at[k], x_peer
            )

        def send_over_x(j):
            if j < chunks:
                wait_loaded(False, j)
                rows = pl.ds(j * _ROWS, _ROWS)
                raw_out[rows, :] = theirs[rows, :].astype(raw_out.dtype)
                if j == 0:
                    pl.when(odd == 0)(lambda: pl.semaphore_wait(barrier, 2))
                    pl.when(odd == 1)(lambda: pl.semaphore_wait(barrier, 1))
                raw_copy(j).start()
                if j == 0:
                    pl.when(odd == 0)(lambda: signal(y_ready, y_peer))
            elif j < chunks + body_chunks:
                k = j - chunks
                own = block(my_x, my_y, k * _ROWS)
                sent = own_x_sent[k * _ROWS // share]
                remote(own, own, sent, sum_sems.at[k], x_peer).start()
            elif j == chunks + body_chunks:
                own = block(my_x, my_y, tail_row, tail_rows)
                remote(own, own, own_x_sent[-1], tail_own, x_peer).start()
                diag = block(my_x, 1 - my_y, tail_row, tail_rows)
                wait_received(diag, tail_over_y)
                remote(diag, diag, tail_sent, tail_diag, x_peer).start()

        for j in range(_AHEAD):
            send_over_x(j)

        for k in range(chunks):
            p, rows = k * _ROWS // share, pl.ds(k * _ROWS, _ROWS)
            wait_loaded(True, k)
            raw_copy(k).wait_recv()
            own = block(my_x, my_y, k * _ROWS)
            total = mine[rows, :] + raw_in[rows, :].astype(mine.dtype)
            own[...] = total.astype(own.dtype)
            received = own_received[p] if k < body_chunks else tail_over_y
            remote(own, own, own_y_sent[p], received, y_peer).start()
            send_over_x(k + _AHEAD)

        for k in range(body_chunks):
            p = k * _ROWS // share
            other = block(1 - my_x, my_y, k * _ROWS)
            wait_received(other, sum_sems.at[k])
            remote(other, other, diag_sent[p], diag_received[p], y_peer).start()
            send_over_x(chunks + k + _AHEAD)

        wait_sent(raw_out, raw_sent)
        for p in range(_PARTS):
            rows = share - (tail_rows if p == _PARTS - 1 else 0)
            wait_sent(block(my_x, my_y, p * share, share), own_y_sent[p])
            wait_received(block(my_x, 1 - my_y, p * share, rows), own_received[p])
            wait_sent(block(my_x, my_y, p * share, share), own_x_sent[p])
            wait_sent(block(1 - my_x, my_y, p * share, rows), diag_sent[p])
            if p == _PARTS - 1:
                wait_sent(block(my_x, 1 - my_y, tail_row, tail_rows), tail_sent)
                wait_received(block(1 - my_x, my_y, tail_row, tail_rows), tail_own)
                wait_received(block(1 - my_x, 1 - my_y, tail_row, tail_rows), tail_diag)
            wait_received(block(1 - my_x, 1 - my_y, p * share, rows), diag_received[p])

    wire = jnp.bfloat16
    blocks = pl.pallas_call(
        kernel,
        out_shape=[pltpu.VMEM((part, 2 * n), wire)] * _PARTS,
        in_specs=[pl.BlockSpec(memory_space=pltpu.HBM)],
        out_specs=[pl.BlockSpec(memory_space=pltpu.VMEM)] * _PARTS,
        scratch_shapes=[
            pltpu.VMEM((half, n), x.dtype),
            pltpu.VMEM((half, n), x.dtype),
            pltpu.VMEM((half, n), wire),
            pltpu.VMEM((half, n), wire),
            pltpu.SemaphoreType.DMA((len(_LOADS),)),
            pltpu.SemaphoreType.DMA((chunks,)),
            pltpu.SemaphoreType.DMA((body_chunks,)),
            pltpu.SemaphoreType.DMA((5, _PARTS)),
            pltpu.SemaphoreType.DMA((5,)),
            pltpu.SemaphoreType.REGULAR,
        ],
        compiler_params=pltpu.CompilerParams(
            collective_id=0,
            vmem_limit_bytes=32 * 1024 * 1024,
            disable_semaphore_checks=True,
        ),
    )(x)
    return jnp.concatenate(blocks, axis=0)
```

```python
import jax
import jax.numpy as jnp
from jax import lax
from jax.experimental import pallas as pl
from jax.experimental.pallas import tpu as pltpu

_ROWS = 8
_AHEAD = 10
_TAIL = 3
_PARTS = 4
_LOADS = (
    (False, 0, 8), (False, 8, 32), (False, 32, 96), (True, 0, 64),
    (False, 96, 256), (True, 64, 256), (False, 256, 512), (True, 256, 512),
    (False, 512, 768), (True, 512, 768), (False, 768, 1024), (True, 768, 1024),
)


def pallas_dist_rsx_agy_m2048_n1024_kernel(x: jax.Array):
    _, m, n = x.shape
    half = m // 2
    part = m // _PARTS
    share = part // 2
    chunks = half // _ROWS
    body_chunks = chunks - _TAIL
    tail_row, tail_rows = body_chunks * _ROWS, _TAIL * _ROWS
    assert half == _LOADS[-1][2] and share % _ROWS == 0

    def kernel(x_hbm, *refs):
        outs = refs[:_PARTS]
        theirs, mine, raw_out, raw_in = refs[_PARTS : _PARTS + 4]
        load_sems, raw_sems, sum_sems, part_sems, sems, y_ready = refs[_PARTS + 4 :]
        raw_sent, tail_sent, tail_over_y, tail_own, tail_diag = (
            sems.at[i] for i in range(5)
        )
        own_x_sent, own_y_sent, diag_sent, own_received, diag_received = (
            [part_sems.at[i, p] for p in range(_PARTS)] for i in range(5)
        )

        my_x, my_y = lax.axis_index("x"), lax.axis_index("y")
        x_peer, y_peer = (1 - my_x, my_y), (my_x, 1 - my_y)
        odd = my_x ^ my_y

        def signal(sem, peer):
            pl.semaphore_signal(
                sem, 1, device_id=peer, device_id_type=pl.DeviceIdType.MESH
            )

        def remote(src, dst, send_sem, recv_sem, peer):
            return pltpu.make_async_remote_copy(
                src, dst, send_sem, recv_sem, peer, pl.DeviceIdType.MESH
            )

        def wait_sent(ref, sem, peer):
            remote(ref, ref, sem, sem, peer).wait_send()

        def wait_received(ref, sem, peer):
            remote(ref, ref, sem, sem, peer).wait_recv()

        def first_row(owner):
            return pl.multiple_of(owner * share, share)

        def block(owner, column_half, row, rows=_ROWS):
            return outs[row // share].at[
                pl.ds(first_row(owner) + row % share, rows),
                pl.ds(pl.multiple_of(column_half * n, n), n),
            ]

        barrier = pltpu.get_barrier_semaphore()
        signal(barrier, x_peer)
        pl.when(odd == 1)(lambda: signal(barrier, y_peer))

        loads = []
        for i, (is_mine, lo, hi) in enumerate(_LOADS):
            owner = my_x if is_mine else 1 - my_x
            row = lo // share * part + first_row(owner) + lo % share
            load = pltpu.make_async_copy(
                x_hbm.at[0, pl.ds(row, hi - lo), :],
                (mine if is_mine else theirs).at[pl.ds(lo, hi - lo), :],
                load_sems.at[i],
            )
            load.start()
            loads.append(load)

        def wait_loaded(is_mine, k):
            for load, (load_is_mine, lo, _) in zip(loads, _LOADS):
                if load_is_mine == is_mine and lo == k * _ROWS:
                    load.wait()

        def raw_copy(k):
            rows = pl.ds(k * _ROWS, _ROWS)
            src, dst = raw_out.at[rows, :], raw_in.at[rows, :]
            return remote(src, dst, raw_sent, raw_sems.at[k], x_peer)

        def send_over_x(j):
            if j < chunks:
                wait_loaded(False, j)
                rows = pl.ds(j * _ROWS, _ROWS)
                raw_out[rows, :] = theirs[rows, :].astype(raw_out.dtype)
                if j == 0:
                    pl.when(odd == 0)(lambda: pl.semaphore_wait(barrier, 2))
                    pl.when(odd == 1)(lambda: pl.semaphore_wait(barrier, 1))
                raw_copy(j).start()
                if j == 0:
                    pl.when(odd == 0)(lambda: signal(y_ready, y_peer))
            elif j < chunks + body_chunks:
                k = j - chunks
                own = block(my_x, my_y, k * _ROWS)
                sent = own_x_sent[k * _ROWS // share]
                remote(own, own, sent, sum_sems.at[k], x_peer).start()
            elif j == chunks + body_chunks:
                own = block(my_x, my_y, tail_row, tail_rows)
                remote(own, own, own_x_sent[-1], tail_own, x_peer).start()
                diag = block(my_x, 1 - my_y, tail_row, tail_rows)
                wait_received(diag, tail_over_y, y_peer)
                remote(diag, diag, tail_sent, tail_diag, x_peer).start()

        for j in range(_AHEAD):
            send_over_x(j)

        for k in range(chunks):
            p, rows = k * _ROWS // share, pl.ds(k * _ROWS, _ROWS)
            wait_loaded(True, k)
            raw_copy(k).wait_recv()
            own = block(my_x, my_y, k * _ROWS)
            total = mine[rows, :] + raw_in[rows, :].astype(mine.dtype)
            own[...] = total.astype(own.dtype)
            if k == 0:
                pl.when(odd == 1)(lambda: pl.semaphore_wait(y_ready, 1))
            received = own_received[p] if k < body_chunks else tail_over_y
            remote(own, own, own_y_sent[p], received, y_peer).start()
            send_over_x(k + _AHEAD)

        for k in range(body_chunks):
            p = k * _ROWS // share
            other = block(1 - my_x, my_y, k * _ROWS)
            wait_received(other, sum_sems.at[k], x_peer)
            remote(other, other, diag_sent[p], diag_received[p], y_peer).start()
            send_over_x(chunks + k + _AHEAD)

        wait_sent(raw_out, raw_sent, x_peer)
        for p in range(_PARTS):
            row, last = p * share, p == _PARTS - 1
            rows = share - tail_rows if last else share
            wait_sent(block(my_x, my_y, row, share), own_y_sent[p], y_peer)
            wait_received(block(my_x, 1 - my_y, row, rows), own_received[p], y_peer)
            wait_sent(block(my_x, my_y, row, share), own_x_sent[p], x_peer)
            wait_sent(block(1 - my_x, my_y, row, rows), diag_sent[p], y_peer)
            if last:
                tail = tail_row, tail_rows
                wait_sent(block(my_x, 1 - my_y, *tail), tail_sent, x_peer)
                wait_received(block(1 - my_x, my_y, *tail), tail_own, x_peer)
                wait_received(block(1 - my_x, 1 - my_y, *tail), tail_diag, x_peer)
            wait_received(
                block(1 - my_x, 1 - my_y, row, rows), diag_received[p], y_peer
            )

    wire = jnp.bfloat16
    blocks = pl.pallas_call(
        kernel,
        out_shape=[pltpu.VMEM((part, 2 * n), wire)] * _PARTS,
        in_specs=[pl.BlockSpec(memory_space=pltpu.HBM)],
        out_specs=[pl.BlockSpec(memory_space=pltpu.VMEM)] * _PARTS,
        scratch_shapes=[
            pltpu.VMEM((half, n), x.dtype),
            pltpu.VMEM((half, n), x.dtype),
            pltpu.VMEM((half, n), wire),
            pltpu.VMEM((half, n), wire),
            pltpu.SemaphoreType.DMA((len(_LOADS),)),
            pltpu.SemaphoreType.DMA((chunks,)),
            pltpu.SemaphoreType.DMA((body_chunks,)),
            pltpu.SemaphoreType.DMA((5, _PARTS)),
            pltpu.SemaphoreType.DMA((5,)),
            pltpu.SemaphoreType.REGULAR,
        ],
        compiler_params=pltpu.CompilerParams(
            collective_id=0,
            vmem_limit_bytes=32 * 1024 * 1024,
            disable_semaphore_checks=True,
        ),
    )(x)
    return jnp.concatenate(blocks, axis=0)
```
